```python
import numpy as np

kernel_name = "dist_argmax_global_i_m8192_n1024"

def setup_inputs():
    return {"x": np.random.randn(32768, 1024).astype(np.float32)}

def reference(x: np.ndarray) -> np.ndarray:
    idx = np.argmax(x, axis=0).astype(np.float32)
    val = np.max(x, axis=0)
    return np.stack([val, idx], axis=0)
```

```python
import jax
import jax.numpy as jnp
from jax import lax
from jax.experimental import pallas as pl
from jax.experimental.pallas import tpu as pltpu

N_DEV = 4
LANES = 128
SUB = 8
MESH = pl.DeviceIdType.MESH

BIG = 512
MID = (256, 192, 128)
TAIL = 128
PIECES = 2
LAST = (96, 16, 16)
REMOTE = (352, 64)
REMOTE_AT = (0, 2)
UNROLL = 8
SEND_ORDER = (2, 1, 3)
WAIT_ORDER = (1, 3, 2)


def _lexmerge(v, i, bv, bi):
    take = (v > bv) | ((v == bv) & (i < bi))
    return jnp.where(take, v, bv), jnp.where(take, i, bi)


def pallas_dist_argmax_global_i_m8192_n1024_kernel(x: jax.Array):
    m, n = x.shape
    ncol = n // LANES
    r_rows = sum(REMOTE)
    l_rows = m - 2 * r_rows
    nbig = (l_rows - TAIL - sum(MID)) // BIG
    assert BIG * nbig + sum(MID) + TAIL == l_rows and sum(LAST) == TAIL
    mid_start = [BIG * nbig + sum(MID[:k]) for k in range(len(MID))]
    rem_start = [sum(REMOTE[:j]) for j in range(len(REMOTE))]
    nrem = len(REMOTE)
    cpp = ncol // PIECES
    wid = cpp * LANES
    t0 = l_rows - TAIL
    tail = [(p, t0, TAIL) for p in range(PIECES - 1)]
    r0 = t0
    for rows in LAST:
        tail.append((PIECES - 1, r0, rows))
        r0 += rows

    def body(x_hbm, out_ref, buf, rbuf, part, gath,
             big_sems, mid_sems, tail_sems, raw_send, raw_recv, send_sems, recv_sems):
        me = lax.axis_index("i")
        right = (me + 1) % N_DEV
        left = (me + N_DEV - 1) % N_DEV

        def big_copy(i):
            s = pl.multiple_of(i * BIG, BIG)
            return pltpu.make_async_copy(
                x_hbm.at[pl.ds(s, BIG)], buf.at[pl.ds(s, BIG)], big_sems.at[i])

        def mid_copy(k):
            rows = pl.ds(mid_start[k], MID[k])
            return pltpu.make_async_copy(x_hbm.at[rows], buf.at[rows], mid_sems.at[k])

        def tail_copy(k):
            p, r, rows = tail[k]
            blk = (pl.ds(r, rows), pl.ds(p * wid, wid))
            return pltpu.make_async_copy(x_hbm.at[blk], buf.at[blk], tail_sems.at[k])

        def raw_copy(side, j):
            s = l_rows + side * r_rows + rem_start[j]
            return pltpu.make_async_remote_copy(
                x_hbm.at[pl.ds(s, REMOTE[j])],
                rbuf.at[side, pl.ds(rem_start[j], REMOTE[j])],
                raw_send.at[side * nrem + j], raw_recv.at[side * nrem + j],
                device_id=(right if side == 0 else left,), device_id_type=MESH)

        big_copy(0).start()
        barrier = pltpu.get_barrier_semaphore()
        for d in range(1, N_DEV):
            pl.semaphore_signal(barrier, inc=1, device_id=((me + d) % N_DEV,),
                                device_id_type=MESH)
        for i in range(1, nbig):
            big_copy(i).start()
        for k in range(len(MID)):
            mid_copy(k).start()
        for k in range(len(tail)):
            tail_copy(k).start()
        pl.semaphore_wait(barrier, N_DEV - 1)
        for j in range(nrem):
            for side in (0, 1):
                raw_copy(side, j).start()

        sub_f = lax.broadcasted_iota(jnp.int32, (SUB, LANES), 0).astype(jnp.float32)

        def groups(ref, row0, count, gidx, mx, ix, cols):
            mx, ix = dict(mx), dict(ix)
            for u in range(count):
                g = gidx + float(SUB * u) if u else gidx
                for c in cols:
                    xv = ref[pl.ds(row0 + SUB * u, SUB), pl.ds(c * LANES, LANES)]
                    better = xv > mx[c]
                    mx[c] = jnp.where(better, xv, mx[c])
                    ix[c] = jnp.where(better, g, ix[c])
            return mx, ix

        def fold(ref, row0, rows, base, mx, ix, cols):
            ngroups = rows // SUB
            row0_f = float(row0) if isinstance(row0, int) else row0.astype(jnp.float32)
            gidx = sub_f + (base + row0_f)
            iters = ngroups // UNROLL
            done = 0
            if iters >= 2:
                def step(t, carry):
                    cm, ci, g = carry
                    r = pl.multiple_of(row0 + t * (SUB * UNROLL), SUB)
                    cm, ci = groups(ref, r, UNROLL, g, cm, ci, cols)
                    return cm, ci, g + float(SUB * UNROLL)

                cm, ci, gidx = lax.fori_loop(
                    0, iters, step,
                    ({c: mx[c] for c in cols}, {c: ix[c] for c in cols}, gidx))
                mx, ix = {**mx, **cm}, {**ix, **ci}
                done = iters * UNROLL
            if ngroups - done:
                mx, ix = groups(ref, row0 + done * SUB, ngroups - done, gidx, mx, ix, cols)
            return mx, ix

        all_cols = list(range(ncol))
        neg_inf = jnp.full((SUB, LANES), -jnp.inf, jnp.float32)

        def fresh(base):
            return {c: neg_inf for c in all_cols}, {c: sub_f + base for c in all_cols}

        my_base = (me * m).astype(jnp.float32)

        def main(i, carry):
            big_copy(i).wait()
            return fold(buf, i * BIG, BIG, my_base, carry[0], carry[1], all_cols)

        mx, ix = lax.fori_loop(0, nbig, main, fresh(my_base))

        rem_base = [(left * m + l_rows).astype(jnp.float32),
                    (right * m + l_rows + r_rows).astype(jnp.float32)]
        rem_acc = [fresh(rem_base[0]), fresh(rem_base[1])]
        for k in range(len(MID) + 1):
            for j in range(nrem):
                if REMOTE_AT[j] == k:
                    for side in (0, 1):
                        raw_copy(side, j).wait_recv()
                        rem_acc[side] = fold(rbuf.at[side], rem_start[j], REMOTE[j],
                                             rem_base[side], *rem_acc[side], all_cols)
            if k < len(MID):
                mid_copy(k).wait()
                mx, ix = fold(buf, mid_start[k], MID[k], my_base, mx, ix, all_cols)
        rem = {c: _lexmerge(rem_acc[0][0][c], rem_acc[0][1][c],
                            rem_acc[1][0][c], rem_acc[1][1][c]) for c in all_cols}

        mine, sent = {}, {}
        for k, (p, r, rows) in enumerate(tail):
            cols = list(range(p * cpp, (p + 1) * cpp))
            tail_copy(k).wait()
            mx, ix = fold(buf, r, rows, my_base, mx, ix, cols)
            if k + 1 < len(tail) and tail[k + 1][0] == p:
                continue
            for cc, c in enumerate(cols):
                v, g = _lexmerge(*rem[c], mx[c], ix[c])
                for shift in (4, 2, 1):
                    v, g = _lexmerge(pltpu.roll(v, shift, 0), pltpu.roll(g, shift, 0), v, g)
                mine[c] = (v[0:1, :], g[0:1, :])
                part[p, 0, :, pl.ds(cc * LANES, LANES)] = mine[c][0]
                part[p, 1, :, pl.ds(cc * LANES, LANES)] = mine[c][1]
            for d in SEND_ORDER:
                s = (d - 1) * PIECES + p
                sent[d, p] = pltpu.make_async_remote_copy(
                    part.at[p], gath.at[d - 1, p], send_sems.at[s], recv_sems.at[s],
                    device_id=((me + d) % N_DEV,), device_id_type=MESH)
                sent[d, p].start()

        for p in range(PIECES):
            cols = list(range(p * cpp, (p + 1) * cpp))
            acc = {c: mine[c] for c in cols}
            for d in WAIT_ORDER:
                sent[d, p].wait_recv()
                for cc, c in enumerate(cols):
                    lanes = pl.ds(cc * LANES, LANES)
                    acc[c] = _lexmerge(gath[d - 1, p, 0, :, lanes], gath[d - 1, p, 1, :, lanes],
                                       *acc[c])
            for c in cols:
                out_ref[0:1, pl.ds(c * LANES, LANES)] = acc[c][0]
                out_ref[1:2, pl.ds(c * LANES, LANES)] = acc[c][1]

        for cpy in sent.values():
            cpy.wait_send()
        for j in range(nrem):
            for side in (0, 1):
                raw_copy(side, j).wait_send()

    return pl.pallas_call(
        body,
        out_shape=jax.ShapeDtypeStruct((2, n), jnp.float32),
        in_specs=[pl.BlockSpec(memory_space=pl.ANY)],
        out_specs=pl.BlockSpec(memory_space=pltpu.VMEM),
        scratch_shapes=[
            pltpu.VMEM((l_rows, n), jnp.float32),
            pltpu.VMEM((2, r_rows, n), jnp.float32),
            pltpu.VMEM((PIECES, 2, 1, wid), jnp.float32),
            pltpu.VMEM((N_DEV - 1, PIECES, 2, 1, wid), jnp.float32),
            pltpu.SemaphoreType.DMA((nbig,)),
            pltpu.SemaphoreType.DMA((len(MID),)),
            pltpu.SemaphoreType.DMA((len(tail),)),
            pltpu.SemaphoreType.DMA((2 * nrem,)),
            pltpu.SemaphoreType.DMA((2 * nrem,)),
            pltpu.SemaphoreType.DMA(((N_DEV - 1) * PIECES,)),
            pltpu.SemaphoreType.DMA(((N_DEV - 1) * PIECES,)),
        ],
        compiler_params=pltpu.CompilerParams(
            vmem_limit_bytes=100 * 1024 * 1024,
            collective_id=0,
            disable_semaphore_checks=True,
        ),
    )(x)
```

```python
import jax
import jax.numpy as jnp
from jax import lax
from jax.experimental import pallas as pl
from jax.experimental.pallas import tpu as pltpu

N_DEV = 4
LANES = 128
SUB = 8
MESH = pl.DeviceIdType.MESH

BIG = 512
MID = (256, 160, 96)
TAIL = 128
PIECES = 4
LAST = (112, 16)
REMOTE = (384, 64)
REMOTE_AT = (1, 3)
UNROLL = 8
SEND_ORDER = (2, 1, 3)
WAIT_ORDER = (1, 3, 2)


def _lexmerge(v, i, bv, bi):
    take = (v > bv) | ((v == bv) & (i < bi))
    return jnp.where(take, v, bv), jnp.where(take, i, bi)


def pallas_dist_argmax_global_i_m8192_n1024_kernel(x: jax.Array):
    m, n = x.shape
    ncol = n // LANES
    r_rows = sum(REMOTE)
    l_rows = m - 2 * r_rows
    nbig = (l_rows - TAIL - sum(MID)) // BIG
    assert BIG * nbig + sum(MID) + TAIL == l_rows and sum(LAST) == TAIL
    mid_start = [BIG * nbig + sum(MID[:k]) for k in range(len(MID))]
    rem_start = [sum(REMOTE[:j]) for j in range(len(REMOTE))]
    nrem = len(REMOTE)
    cpp = ncol // PIECES
    wid = cpp * LANES
    t0 = l_rows - TAIL
    tail = [(p, t0, TAIL) for p in range(PIECES - 1)]
    r0 = t0
    for rows in LAST:
        tail.append((PIECES - 1, r0, rows))
        r0 += rows

    def body(x_hbm, out_ref, buf, rbuf, part, gath,
             big_sems, mid_sems, tail_sems, raw_send, raw_recv, send_sems, recv_sems):
        me = lax.axis_index("i")
        right = (me + 1) % N_DEV
        left = (me + N_DEV - 1) % N_DEV

        def big_copy(i):
            s = pl.multiple_of(i * BIG, BIG)
            return pltpu.make_async_copy(
                x_hbm.at[pl.ds(s, BIG)], buf.at[pl.ds(s, BIG)], big_sems.at[i])

        def mid_copy(k):
            rows = pl.ds(mid_start[k], MID[k])
            return pltpu.make_async_copy(x_hbm.at[rows], buf.at[rows], mid_sems.at[k])

        def tail_copy(k):
            p, r, rows = tail[k]
            blk = (pl.ds(r, rows), pl.ds(p * wid, wid))
            return pltpu.make_async_copy(x_hbm.at[blk], buf.at[blk], tail_sems.at[k])

        def raw_copy(side, j):
            s = l_rows + side * r_rows + rem_start[j]
            return pltpu.make_async_remote_copy(
                x_hbm.at[pl.ds(s, REMOTE[j])],
                rbuf.at[side, pl.ds(rem_start[j], REMOTE[j])],
                raw_send.at[side * nrem + j], raw_recv.at[side * nrem + j],
                device_id=(right if side == 0 else left,), device_id_type=MESH)

        big_copy(0).start()
        barrier = pltpu.get_barrier_semaphore()
        for d in range(1, N_DEV):
            pl.semaphore_signal(barrier, inc=1, device_id=((me + d) % N_DEV,),
                                device_id_type=MESH)
        for i in range(1, nbig):
            big_copy(i).start()
        for k in range(len(MID)):
            mid_copy(k).start()
        for k in range(len(tail)):
            tail_copy(k).start()
        pl.semaphore_wait(barrier, N_DEV - 1)
        for j in range(nrem):
            for side in (0, 1):
                raw_copy(side, j).start()

        sub_f = lax.broadcasted_iota(jnp.int32, (SUB, LANES), 0).astype(jnp.float32)

        def groups(ref, row0, count, gidx, mx, ix, cols):
            mx, ix = dict(mx), dict(ix)
            for u in range(count):
                g = gidx + float(SUB * u) if u else gidx
                for c in cols:
                    xv = ref[pl.ds(row0 + SUB * u, SUB), pl.ds(c * LANES, LANES)]
                    better = xv > mx[c]
                    mx[c] = jnp.where(better, xv, mx[c])
                    ix[c] = jnp.where(better, g, ix[c])
            return mx, ix

        def fold(ref, row0, rows, base, mx, ix, cols):
            ngroups = rows // SUB
            row0_f = float(row0) if isinstance(row0, int) else row0.astype(jnp.float32)
            gidx = sub_f + (base + row0_f)
            iters = ngroups // UNROLL
            done = 0
            if iters >= 2:
                def step(t, carry):
                    cm, ci, g = carry
                    r = pl.multiple_of(row0 + t * (SUB * UNROLL), SUB)
                    cm, ci = groups(ref, r, UNROLL, g, cm, ci, cols)
                    return cm, ci, g + float(SUB * UNROLL)

                cm, ci, gidx = lax.fori_loop(
                    0, iters, step,
                    ({c: mx[c] for c in cols}, {c: ix[c] for c in cols}, gidx))
                mx, ix = {**mx, **cm}, {**ix, **ci}
                done = iters * UNROLL
            if ngroups - done:
                mx, ix = groups(ref, row0 + done * SUB, ngroups - done, gidx, mx, ix, cols)
            return mx, ix

        all_cols = list(range(ncol))
        neg_inf = jnp.full((SUB, LANES), -jnp.inf, jnp.float32)

        def fresh(base):
            return {c: neg_inf for c in all_cols}, {c: sub_f + base for c in all_cols}

        my_base = (me * m).astype(jnp.float32)

        def main(i, carry):
            big_copy(i).wait()
            return fold(buf, i * BIG, BIG, my_base, carry[0], carry[1], all_cols)

        mx, ix = lax.fori_loop(0, nbig, main, fresh(my_base))

        rem_base = [(left * m + l_rows).astype(jnp.float32),
                    (right * m + l_rows + r_rows).astype(jnp.float32)]
        rem_acc = [fresh(rem_base[0]), fresh(rem_base[1])]
        for k in range(len(MID) + 1):
            for j in range(nrem):
                if REMOTE_AT[j] == k:
                    for side in (0, 1):
                        raw_copy(side, j).wait_recv()
                        rem_acc[side] = fold(rbuf.at[side], rem_start[j], REMOTE[j],
                                             rem_base[side], *rem_acc[side], all_cols)
            if k < len(MID):
                mid_copy(k).wait()
                mx, ix = fold(buf, mid_start[k], MID[k], my_base, mx, ix, all_cols)
        rem = {c: _lexmerge(rem_acc[0][0][c], rem_acc[0][1][c],
                            rem_acc[1][0][c], rem_acc[1][1][c]) for c in all_cols}
        for j in range(nrem):
            for side in (0, 1):
                raw_copy(side, j).wait_send()

        mine, sent = {}, {}
        for k, (p, r, rows) in enumerate(tail):
            cols = list(range(p * cpp, (p + 1) * cpp))
            tail_copy(k).wait()
            mx, ix = fold(buf, r, rows, my_base, mx, ix, cols)
            if k + 1 < len(tail) and tail[k + 1][0] == p:
                continue
            for cc, c in enumerate(cols):
                v, g = _lexmerge(*rem[c], mx[c], ix[c])
                for shift in (4, 2, 1):
                    v, g = _lexmerge(pltpu.roll(v, shift, 0), pltpu.roll(g, shift, 0), v, g)
                mine[c] = (v[0:1, :], g[0:1, :])
                part[p, 0, :, pl.ds(cc * LANES, LANES)] = mine[c][0]
                part[p, 1, :, pl.ds(cc * LANES, LANES)] = mine[c][1]
            for d in SEND_ORDER:
                s = (d - 1) * PIECES + p
                sent[d, p] = pltpu.make_async_remote_copy(
                    part.at[p], gath.at[d - 1, p], send_sems.at[s], recv_sems.at[s],
                    device_id=((me + d) % N_DEV,), device_id_type=MESH)
                sent[d, p].start()

        for p in range(PIECES):
            cols = list(range(p * cpp, (p + 1) * cpp))
            acc = {c: mine[c] for c in cols}
            for d in WAIT_ORDER:
                if p == PIECES - 1 and d == WAIT_ORDER[-1]:
                    for cpy in sent.values():
                        cpy.wait_send()
                sent[d, p].wait_recv()
                for cc, c in enumerate(cols):
                    lanes = pl.ds(cc * LANES, LANES)
                    acc[c] = _lexmerge(gath[d - 1, p, 0, :, lanes], gath[d - 1, p, 1, :, lanes],
                                       *acc[c])
            for c in cols:
                out_ref[0:1, pl.ds(c * LANES, LANES)] = acc[c][0]
                out_ref[1:2, pl.ds(c * LANES, LANES)] = acc[c][1]

    return pl.pallas_call(
        body,
        out_shape=jax.ShapeDtypeStruct((2, n), jnp.float32),
        in_specs=[pl.BlockSpec(memory_space=pl.ANY)],
        out_specs=pl.BlockSpec(memory_space=pltpu.VMEM),
        scratch_shapes=[
            pltpu.VMEM((l_rows, n), jnp.float32),
            pltpu.VMEM((2, r_rows, n), jnp.float32),
            pltpu.VMEM((PIECES, 2, 1, wid), jnp.float32),
            pltpu.VMEM((N_DEV - 1, PIECES, 2, 1, wid), jnp.float32),
            pltpu.SemaphoreType.DMA((nbig,)),
            pltpu.SemaphoreType.DMA((len(MID),)),
            pltpu.SemaphoreType.DMA((len(tail),)),
            pltpu.SemaphoreType.DMA((2 * nrem,)),
            pltpu.SemaphoreType.DMA((2 * nrem,)),
            pltpu.SemaphoreType.DMA(((N_DEV - 1) * PIECES,)),
            pltpu.SemaphoreType.DMA(((N_DEV - 1) * PIECES,)),
        ],
        compiler_params=pltpu.CompilerParams(
            vmem_limit_bytes=100 * 1024 * 1024,
            collective_id=0,
            disable_semaphore_checks=True,
        ),
    )(x)
```
